```python
import numpy as np

kernel_name = "dist_ar_xy_y_m256_n256"

def setup_inputs():
    return {"x": np.random.randn(512, 256).astype(np.float32)}

def reference(x: np.ndarray) -> np.ndarray:
    return x.reshape(2, 256, 256).sum(axis=0)
```

```python
import jax
import jax.numpy as jnp
from jax import lax
from jax.experimental import pallas as pl
from jax.experimental.pallas import tpu as pltpu


def pallas_dist_ar_xy_y_m256_n256_kernel(
x: jax.Array,
):
    m, n = x.shape

    def kernel_body(x_ref, out_ref, send_buf, recv_buf, send_sem, recv_sem):
        my_x = lax.axis_index("x")
        my_y = lax.axis_index("y")
        peer = (my_x, 1 - my_y)

        barrier_sem = pltpu.get_barrier_semaphore()
        pl.semaphore_signal(
            barrier_sem, inc=1, device_id=peer,
            device_id_type=pl.DeviceIdType.MESH)
        send_buf[...] = x_ref[...].astype(jnp.bfloat16)
        pl.semaphore_wait(barrier_sem, 1)

        rdma = pltpu.make_async_remote_copy(
            src_ref=send_buf, dst_ref=recv_buf,
            send_sem=send_sem, recv_sem=recv_sem,
            device_id=peer, device_id_type=pl.DeviceIdType.MESH)
        rdma.start()
        rdma.wait_recv()
        out_ref[...] = x_ref[...] + recv_buf[...].astype(jnp.float32)
        rdma.wait_send()

    return pl.pallas_call(
        kernel_body,
        out_shape=jax.ShapeDtypeStruct((m, n), jnp.float32),
        in_specs=[pl.BlockSpec(memory_space=pltpu.VMEM)],
        out_specs=pl.BlockSpec(memory_space=pltpu.VMEM),
        scratch_shapes=[
            pltpu.VMEM((m, n), jnp.bfloat16),
            pltpu.VMEM((m, n), jnp.bfloat16),
            pltpu.SemaphoreType.DMA,
            pltpu.SemaphoreType.DMA,
        ],
        compiler_params=pltpu.CompilerParams(collective_id=0),
    )(x)
```

```python
import jax
import jax.numpy as jnp
from jax import lax
from jax.experimental import pallas as pl
from jax.experimental.pallas import tpu as pltpu

_LANES = 128
_TILE = 8
_BAND = 16
_ROWS = 512


def _spans(*cuts):
    return tuple((lo, hi - lo) for lo, hi in zip(cuts, cuts[1:]))


_RELAY_END = 104
_DIRECT_F32 = 488
_LAST_BAND = _RELAY_END // _BAND * _BAND

_RELAY_F32 = _spans(0, 8, 12, 14, 16)
_RELAY_BF16 = _spans(*range(16, _RELAY_END + 1, 2))
_RELAY_LOADS_EARLY = _spans(16, 24, 32, 40, 48, 64, 80, 112)
_RELAY_LOADS_LATE = _spans(112, 176, 304, _ROWS) + _spans(0, 16)
_RELAY_REST = _spans(_RELAY_END, 112, 176, 304, 448, 496, _ROWS)

_DIRECT_HEAD = _spans(*range(_DIRECT_F32, _ROWS + 1, _TILE))
_DIRECT_LOADS_EARLY = _spans(112, 120, 128, 136, 144, 160, 176, 208, 320)
_DIRECT_LOADS_LATE = _spans(320, _ROWS) + _spans(0, 112)
_DIRECT_BF16 = (
    _spans(112, 120, 128, 136, 144, 160, 176, 208, 320, 448, _DIRECT_F32)
    + _spans(_RELAY_END, 112)
)

_BACK_RELAY, _BACK_DIRECT = _spans(0, 96, _ROWS)

_N_LOADS = max(
    len(_RELAY_LOADS_EARLY + _RELAY_LOADS_LATE),
    len(_DIRECT_LOADS_EARLY + _DIRECT_LOADS_LATE),
)
_N_RELAY = len(_RELAY_F32 + _RELAY_BF16)
_N_STREAM = max(len(_RELAY_REST), len(_DIRECT_HEAD + _DIRECT_BF16))


def _shard_window(start, rows):
    tile, offset = divmod(start, _TILE)
    if offset + rows <= _TILE:
        return (
            pl.ds(_TILE * (tile // 2) + offset, rows),
            pl.ds(_LANES * (tile % 2), _LANES),
        )
    assert start % _BAND == 0 and rows % _BAND == 0
    return pl.ds(start // 2, rows // 2), slice(None)


def _kernel_body(
    x_hbm,
    out,
    tx_buf,
    rx_buf,
    f32_buf,
    load_sems,
    relay_tx, relay_rx,
    stream_tx, stream_rx,
    back_tx, back_rx,
):
    my_x = lax.axis_index("x")
    my_y = lax.axis_index("y")
    barrier = pltpu.get_barrier_semaphore()

    def entered(peer):
        pl.semaphore_signal(
            barrier, inc=1, device_id=peer,
            device_id_type=pl.DeviceIdType.MESH)

    def remote(src, dst, tx_sems, rx_sems, i, peer):
        return pltpu.make_async_remote_copy(
            src_ref=src, dst_ref=dst,
            send_sem=tx_sems.at[i], recv_sem=rx_sems.at[i],
            device_id=peer, device_id_type=pl.DeviceIdType.MESH)

    def bf16_copies(src, spans, tx_sems, rx_sems, peer, first=0):
        return [
            remote(src.at[pl.ds(*s)], rx_buf.at[pl.ds(*s)],
                   tx_sems, rx_sems, first + i, peer)
            for i, s in enumerate(spans)
        ]

    def f32_copies(spans, tx_sems, rx_sems, peer):
        base = spans[0][0]
        return [
            remote(x_hbm.at[_shard_window(start, rows)],
                   f32_buf.at[pl.ds(start - base, rows)],
                   tx_sems, rx_sems, i, peer)
            for i, (start, rows) in enumerate(spans)
        ]

    def loads(spans, first=0):
        return [
            pltpu.make_async_copy(
                x_hbm.at[_shard_window(*s)], out.at[_shard_window(*s)],
                load_sems.at[first + i])
            for i, s in enumerate(spans)
        ]

    def pack(start, rows):
        end = start + rows
        while start < end:
            if start % _BAND == 0 and start + _BAND <= end:
                band = out[_shard_window(start, _BAND)]
                value = jnp.concatenate(
                    [band[:, :_LANES], band[:, _LANES:]], axis=0)
            else:
                value = out[_shard_window(start, _TILE)]
            tx_buf[pl.ds(start, value.shape[0]), :] = value.astype(jnp.bfloat16)
            start += value.shape[0]

    def round_f32(start, rows, base):
        rx_buf[pl.ds(start, rows), :] = (
            f32_buf[pl.ds(start - base, rows), :].astype(jnp.bfloat16))

    def add(start, end):
        for row in range(start, end, _BAND):
            other = rx_buf[pl.ds(row, _BAND), :].astype(jnp.float32)
            window = _shard_window(row, _BAND)
            out[window] = out[window] + jnp.concatenate(
                [other[:_TILE], other[_TILE:]], axis=1)

    def stream(sends, spans, early, late, load_spans):
        pending = list(zip(early + late, load_spans, strict=True))
        loaded, packed = set(), set()
        for i, (send, (start, rows)) in enumerate(zip(sends, spans, strict=True)):
            tiles = set(range(start // _TILE, pl.cdiv(start + rows, _TILE)))
            while not tiles <= loaded:
                load, (lo, n) = pending.pop(0)
                load.wait()
                loaded |= set(range(lo // _TILE, (lo + n) // _TILE))
            todo = sorted(tiles - packed)
            if todo:
                lo, hi = todo[0], todo[-1] + 1
                if hi % 2 and hi in loaded - packed:
                    hi += 1
                pack(lo * _TILE, (hi - lo) * _TILE)
                packed |= set(range(lo, hi))
            send.start()
            if i == 0:
                for load in late:
                    load.start()
        for load, _ in pending:
            load.wait()

    def load_shard():
        (load,) = loads([(0, _ROWS)])
        load.start()
        load.wait()

    def direct_from_01():
        peer = (0, 0)
        return (
            f32_copies(_DIRECT_HEAD, stream_tx, stream_rx, peer),
            bf16_copies(tx_buf, _DIRECT_BF16, stream_tx, stream_rx, peer,
                        first=len(_DIRECT_HEAD)),
        )

    def stream_from_11():
        peer = (1, 0)
        return (
            f32_copies(_RELAY_F32, relay_tx, relay_rx, peer),
            bf16_copies(tx_buf, _RELAY_BF16, relay_tx, relay_rx, peer,
                        first=len(_RELAY_F32)),
            bf16_copies(tx_buf, _RELAY_REST, stream_tx, stream_rx, peer),
        )

    def relay_from_10():
        return bf16_copies(
            rx_buf, _RELAY_F32 + _RELAY_BF16, relay_tx, relay_rx, (0, 0))

    def back_from_00():
        (copy,) = bf16_copies(
            tx_buf, [_BACK_DIRECT], back_tx, back_rx, (0, 1), first=1)
        return copy

    def back_from_10():
        return bf16_copies(
            tx_buf, [_BACK_RELAY, _BACK_DIRECT], back_tx, back_rx, (1, 1))

    def relay_from_11():
        (copy,) = bf16_copies(rx_buf, [_BACK_RELAY], back_tx, back_rx, (0, 1))
        return copy

    entered((my_x, 1 - my_y))

    @pl.when(jnp.logical_and(my_x == 0, my_y == 1))
    def _chip_01():
        entered((1, 1))
        head, body = direct_from_01()
        early = loads(_DIRECT_LOADS_EARLY)
        late = loads(_DIRECT_LOADS_LATE, first=len(early))
        pl.semaphore_wait(barrier, 1)
        for copy in head + early:
            copy.start()
        stream(body, _DIRECT_BF16, early, late,
               _DIRECT_LOADS_EARLY + _DIRECT_LOADS_LATE)
        for copy in head + body:
            copy.wait_send()
        back_from_00().wait_recv()
        add(_BACK_DIRECT[0], _ROWS)
        relay_from_11().wait_recv()
        add(0, _BACK_DIRECT[0])

    @pl.when(jnp.logical_and(my_x == 1, my_y == 1))
    def _chip_11():
        head, relayed, rest = stream_from_11()
        early = loads(_RELAY_LOADS_EARLY)
        late = loads(_RELAY_LOADS_LATE, first=len(early))
        for load in early:
            load.start()
        pl.semaphore_wait(barrier, 2)
        for copy in head:
            copy.start()
        stream(relayed + rest, _RELAY_BF16 + _RELAY_REST, early, late,
               _RELAY_LOADS_EARLY + _RELAY_LOADS_LATE)
        to_relay, direct = back_from_10()
        relay = relay_from_11()
        to_relay.wait_recv()
        relay.start()
        add(0, _BACK_DIRECT[0])
        for copy in head + relayed + rest + [relay]:
            copy.wait_send()
        direct.wait_recv()
        add(_BACK_DIRECT[0], _ROWS)

    @pl.when(jnp.logical_and(my_x == 1, my_y == 0))
    def _chip_10():
        load_shard()
        pack(0, _ROWS)
        pl.semaphore_wait(barrier, 2)
        back = back_from_10()
        for copy in back:
            copy.start()
        head, relayed, rest = stream_from_11()
        relays = relay_from_10()
        for i, (copy, relay) in enumerate(zip(head + relayed, relays, strict=True)):
            copy.wait_recv()
            if i < len(head):
                round_f32(*_RELAY_F32[i], base=0)
            relay.start()
        done = _LAST_BAND
        add(0, done)
        for copy, (start, rows) in zip(rest, _RELAY_REST, strict=True):
            if copy is rest[-1]:
                for sent in relays + back:
                    sent.wait_send()
            copy.wait_recv()
            add(done, start + rows)
            done = start + rows

    @pl.when(jnp.logical_and(my_x == 0, my_y == 0))
    def _chip_00():
        entered((1, 0))
        load_shard()
        pack(*_BACK_DIRECT)
        pl.semaphore_wait(barrier, 1)
        back = back_from_00()
        back.start()
        head, body = direct_from_01()
        relays = relay_from_10()
        n_first = sum(start < _LAST_BAND for start, _ in _RELAY_F32 + _RELAY_BF16)
        for copy in head:
            copy.wait_recv()
        round_f32(_DIRECT_F32, _ROWS - _DIRECT_F32, base=_DIRECT_F32)
        for copy in body[:-2]:
            copy.wait_recv()
        add(_LAST_BAND + _BAND, _DIRECT_BF16[-2][0])
        back.wait_send()
        for relay in relays[:n_first]:
            relay.wait_recv()
        add(0, _LAST_BAND)
        body[-2].wait_recv()
        add(_DIRECT_BF16[-2][0], _ROWS)
        for copy in [body[-1]] + relays[n_first:]:
            copy.wait_recv()
        add(_LAST_BAND, _LAST_BAND + _BAND)


def pallas_dist_ar_xy_y_m256_n256_kernel(x: jax.Array):
    assert x.shape == (_ROWS // 2, 2 * _LANES) and x.dtype == jnp.float32
    dma_sems = lambda n: pltpu.SemaphoreType.DMA((n,))
    return pl.pallas_call(
        _kernel_body,
        out_shape=jax.ShapeDtypeStruct(x.shape, x.dtype),
        in_specs=[pl.BlockSpec(memory_space=pltpu.HBM)],
        out_specs=pl.BlockSpec(memory_space=pltpu.VMEM),
        scratch_shapes=[
            pltpu.VMEM((_ROWS, _LANES), jnp.bfloat16),
            pltpu.VMEM((_ROWS, _LANES), jnp.bfloat16),
            pltpu.VMEM((_ROWS - _DIRECT_F32, _LANES), jnp.float32),
            dma_sems(_N_LOADS),
            dma_sems(_N_RELAY), dma_sems(_N_RELAY),
            dma_sems(_N_STREAM), dma_sems(_N_STREAM),
            dma_sems(2), dma_sems(2),
        ],
        compiler_params=pltpu.CompilerParams(
            collective_id=0,
            disable_semaphore_checks=True,
        ),
    )(x)
```

```python
import jax
import jax.numpy as jnp
from jax import lax
from jax.experimental import pallas as pl
from jax.experimental.pallas import tpu as pltpu

_LANES = 128
_TILE = 8
_BAND = 16
_ROWS = 512


def _spans(*cuts):
    return tuple((lo, hi - lo) for lo, hi in zip(cuts, cuts[1:]))


_RELAY_END = 106
_DIRECT_F32 = 488
_LAST_BAND = _RELAY_END // _BAND * _BAND

_RELAY_F32 = _spans(*range(0, 17, 2))
_RELAY_BF16 = _spans(*range(16, _RELAY_END + 1, 2))
_RELAY_REST = _spans(_RELAY_END, 112, 176, 304, 448, 496, _ROWS)
_RELAY_LOADS_EARLY = _spans(16, 24, 32, 40, 48, 64, 80, 112)
_RELAY_LOADS_LATE = _spans(112, 176, 304, _ROWS) + _spans(0, 16)

_DIRECT_HEAD = _spans(*range(_DIRECT_F32, _ROWS + 1, _TILE))
_DIRECT_BF16 = (
    _spans(112, 120, 128, 136, 144, 160, 176, 208, 320, 448, _DIRECT_F32)
    + _spans(_RELAY_END, 112)
)
_DIRECT_LOADS_EARLY = _spans(112, 120, 128, 136, 144, 160, 176, 208, 320)
_DIRECT_LOADS_LATE = _spans(320, _ROWS) + _spans(0, 112)

_BACK_RELAY, _BACK_DIRECT = _spans(0, 96, _ROWS)

_N_LOADS = max(
    len(_RELAY_LOADS_EARLY + _RELAY_LOADS_LATE),
    len(_DIRECT_LOADS_EARLY + _DIRECT_LOADS_LATE),
)
_N_RELAY = len(_RELAY_F32 + _RELAY_BF16)
_N_STREAM = max(len(_RELAY_REST), len(_DIRECT_HEAD + _DIRECT_BF16))


def _shard_window(start, rows):
    tile, offset = divmod(start, _TILE)
    if offset + rows <= _TILE:
        return (
            pl.ds(_TILE * (tile // 2) + offset, rows),
            pl.ds(_LANES * (tile % 2), _LANES),
        )
    assert start % _BAND == 0 and rows % _BAND == 0
    return pl.ds(start // 2, rows // 2), slice(None)


def _kernel_body(
    x_hbm,
    out,
    tx_buf,
    rx_buf,
    f32_buf,
    load_sems,
    relay_tx, relay_rx,
    stream_tx, stream_rx,
    back_tx, back_rx,
):
    my_x = lax.axis_index("x")
    my_y = lax.axis_index("y")
    barrier = pltpu.get_barrier_semaphore()

    def entered(peer):
        pl.semaphore_signal(
            barrier, inc=1, device_id=peer,
            device_id_type=pl.DeviceIdType.MESH)

    def remote(src, dst, tx_sems, rx_sems, i, peer):
        return pltpu.make_async_remote_copy(
            src_ref=src, dst_ref=dst,
            send_sem=tx_sems.at[i], recv_sem=rx_sems.at[i],
            device_id=peer, device_id_type=pl.DeviceIdType.MESH)

    def bf16_copies(src, spans, tx_sems, rx_sems, peer, first=0):
        return [
            remote(src.at[pl.ds(*span)], rx_buf.at[pl.ds(*span)],
                   tx_sems, rx_sems, first + i, peer)
            for i, span in enumerate(spans)
        ]

    def f32_copies(spans, tx_sems, rx_sems, peer):
        base = spans[0][0]
        return [
            remote(x_hbm.at[_shard_window(start, rows)],
                   f32_buf.at[pl.ds(start - base, rows)],
                   tx_sems, rx_sems, i, peer)
            for i, (start, rows) in enumerate(spans)
        ]

    def loads(spans, first=0):
        return [
            pltpu.make_async_copy(
                x_hbm.at[_shard_window(*span)], out.at[_shard_window(*span)],
                load_sems.at[first + i])
            for i, span in enumerate(spans)
        ]

    def pack(start, rows):
        if rows == _TILE:
            tile = out[_shard_window(start, _TILE)]
            tx_buf[pl.ds(start, _TILE), :] = tile.astype(jnp.bfloat16)
            return
        for row in range(start, start + rows, _BAND):
            band = out[_shard_window(row, _BAND)]
            tiles = jnp.concatenate([band[:, :_LANES], band[:, _LANES:]], axis=0)
            tx_buf[pl.ds(row, _BAND), :] = tiles.astype(jnp.bfloat16)

    def round_f32(start, rows, base):
        rx_buf[pl.ds(start, rows), :] = (
            f32_buf[pl.ds(start - base, rows), :].astype(jnp.bfloat16))

    def add(start, end):
        for row in range(start, end, _BAND):
            tiles = rx_buf[pl.ds(row, _BAND), :].astype(jnp.float32)
            window = _shard_window(row, _BAND)
            out[window] = out[window] + jnp.concatenate(
                [tiles[:_TILE], tiles[_TILE:]], axis=1)

    def stream(sends, spans, early, late, load_spans):
        for load, (lo, n) in zip(early + late, load_spans, strict=True):
            load.wait()
            ready = [
                send for send, (start, _) in zip(sends, spans, strict=True)
                if lo <= start < lo + n
            ]
            if ready:
                pack(lo, n)
            for send in ready:
                send.start()
                if send is sends[0]:
                    for other in late:
                        other.start()

    def load_shard():
        (load,) = loads([(0, _ROWS)])
        load.start()
        load.wait()

    def direct_from_01():
        return (
            f32_copies(_DIRECT_HEAD, stream_tx, stream_rx, (0, 0)),
            bf16_copies(tx_buf, _DIRECT_BF16, stream_tx, stream_rx, (0, 0),
                        first=len(_DIRECT_HEAD)),
        )

    def stream_from_11():
        return (
            f32_copies(_RELAY_F32, relay_tx, relay_rx, (1, 0)),
            bf16_copies(tx_buf, _RELAY_BF16, relay_tx, relay_rx, (1, 0),
                        first=len(_RELAY_F32)),
            bf16_copies(tx_buf, _RELAY_REST, stream_tx, stream_rx, (1, 0)),
        )

    def relay_from_10():
        return bf16_copies(
            rx_buf, _RELAY_F32 + _RELAY_BF16, relay_tx, relay_rx, (0, 0))

    def back_from_00():
        (copy,) = bf16_copies(
            tx_buf, [_BACK_DIRECT], back_tx, back_rx, (0, 1), first=1)
        return copy

    def back_from_10():
        return bf16_copies(
            tx_buf, [_BACK_RELAY, _BACK_DIRECT], back_tx, back_rx, (1, 1))

    def relay_from_11():
        (copy,) = bf16_copies(rx_buf, [_BACK_RELAY], back_tx, back_rx, (0, 1))
        return copy

    entered((my_x, 1 - my_y))

    @pl.when(jnp.logical_and(my_x == 0, my_y == 1))
    def _chip_01():
        entered((1, 1))
        head, body = direct_from_01()
        early = loads(_DIRECT_LOADS_EARLY)
        late = loads(_DIRECT_LOADS_LATE, first=len(early))
        pl.semaphore_wait(barrier, 1)
        for copy in head + early:
            copy.start()
        stream(body, _DIRECT_BF16, early, late,
               _DIRECT_LOADS_EARLY + _DIRECT_LOADS_LATE)
        for copy in head + body:
            copy.wait_send()
        back_from_00().wait_recv()
        add(_BACK_DIRECT[0], _ROWS)
        relay_from_11().wait_recv()
        add(0, _BACK_DIRECT[0])

    @pl.when(jnp.logical_and(my_x == 1, my_y == 1))
    def _chip_11():
        head, relayed, rest = stream_from_11()
        early = loads(_RELAY_LOADS_EARLY)
        late = loads(_RELAY_LOADS_LATE, first=len(early))
        for load in early:
            load.start()
        pl.semaphore_wait(barrier, 2)
        for copy in head:
            copy.start()
        stream(relayed + rest, _RELAY_BF16 + _RELAY_REST, early, late,
               _RELAY_LOADS_EARLY + _RELAY_LOADS_LATE)
        to_relay, direct = back_from_10()
        relay = relay_from_11()
        to_relay.wait_recv()
        relay.start()
        add(0, _BACK_DIRECT[0])
        for copy in head + relayed + rest + [relay]:
            copy.wait_send()
        direct.wait_recv()
        add(_BACK_DIRECT[0], _ROWS)

    @pl.when(jnp.logical_and(my_x == 1, my_y == 0))
    def _chip_10():
        load_shard()
        pack(0, _ROWS)
        pl.semaphore_wait(barrier, 2)
        back = back_from_10()
        for copy in back:
            copy.start()
        head, relayed, rest = stream_from_11()
        relays = relay_from_10()
        for i, (copy, relay) in enumerate(zip(head + relayed, relays, strict=True)):
            copy.wait_recv()
            if i < len(head):
                round_f32(*_RELAY_F32[i], base=0)
            relay.start()
        done = _LAST_BAND
        add(0, done)
        for copy, (start, rows) in zip(rest, _RELAY_REST, strict=True):
            if copy is rest[-3]:
                for relay in relays:
                    relay.wait_send()
            if copy is rest[-1]:
                for sent in back:
                    sent.wait_send()
            copy.wait_recv()
            add(done, start + rows)
            done = start + rows

    @pl.when(jnp.logical_and(my_x == 0, my_y == 0))
    def _chip_00():
        entered((1, 0))
        load_shard()
        pack(*_BACK_DIRECT)
        pl.semaphore_wait(barrier, 1)
        back = back_from_00()
        back.start()
        head, body = direct_from_01()
        relays = relay_from_10()
        n_first = sum(start < _LAST_BAND for start, _ in _RELAY_F32 + _RELAY_BF16)
        for copy in head:
            copy.wait_recv()
        round_f32(_DIRECT_F32, _ROWS - _DIRECT_F32, base=_DIRECT_F32)
        for copy in body[:-2]:
            copy.wait_recv()
        add(_LAST_BAND + _BAND, _DIRECT_BF16[-2][0])
        back.wait_send()
        for relay in relays[:n_first]:
            relay.wait_recv()
        add(0, _LAST_BAND)
        body[-2].wait_recv()
        add(_DIRECT_BF16[-2][0], _ROWS)
        for copy in [body[-1]] + relays[n_first:]:
            copy.wait_recv()
        add(_LAST_BAND, _LAST_BAND + _BAND)


def pallas_dist_ar_xy_y_m256_n256_kernel(x: jax.Array):
    assert x.shape == (_ROWS // 2, 2 * _LANES) and x.dtype == jnp.float32
    dma_sems = lambda n: pltpu.SemaphoreType.DMA((n,))
    return pl.pallas_call(
        _kernel_body,
        out_shape=jax.ShapeDtypeStruct(x.shape, x.dtype),
        in_specs=[pl.BlockSpec(memory_space=pltpu.HBM)],
        out_specs=pl.BlockSpec(memory_space=pltpu.VMEM),
        scratch_shapes=[
            pltpu.VMEM((_ROWS, _LANES), jnp.bfloat16),
            pltpu.VMEM((_ROWS, _LANES), jnp.bfloat16),
            pltpu.VMEM((_ROWS - _DIRECT_F32, _LANES), jnp.float32),
            dma_sems(_N_LOADS),
            dma_sems(_N_RELAY), dma_sems(_N_RELAY),
            dma_sems(_N_STREAM), dma_sems(_N_STREAM),
            dma_sems(2), dma_sems(2),
        ],
        compiler_params=pltpu.CompilerParams(
            collective_id=0,
            disable_semaphore_checks=True,
        ),
    )(x)
```
